```python
import numpy as np

kernel_name = "dist_sparse_attn_blocksparse_qseq_b2_sq256_skv256_hq4_dh64"

def setup_inputs():
    x = np.random.randn(2, 1024, 512).astype(np.float32)
    Wq = np.random.randn(512, 1024).astype(np.float32) * 0.02
    K_ext = np.random.randn(2, 256, 16, 64).astype(np.float32)
    V_ext = np.random.randn(2, 256, 16, 64).astype(np.float32)
    Wo = np.random.randn(1024, 512).astype(np.float32) * 0.02
    return {"x": x, "Wq": Wq, "K_ext": K_ext, "V_ext": V_ext, "Wo": Wo}

def reference(x, Wq, K_ext, V_ext, Wo):
    B, Sq, Skv, Hq, Dh = 2, 1024, 256, 16, 64
    Q = (x @ Wq).reshape(B, Sq, Hq, Dh)
    qb = (np.arange(Sq) // 64)[:, None]
    kb = (np.arange(Skv) // 64)[None, :]
    mask = (qb == kb) | (kb == 0) | ((qb + kb) % 3 == 0)
    scores = np.einsum('bihd,bjhd->bhij', Q, K_ext).astype(np.float32) * 0.125
    scores = np.where(mask[None, None, :, :], scores, -1e9)
    scores_max = scores.max(axis=-1, keepdims=True)
    w = np.exp(scores - scores_max)
    row_keep = mask.any(axis=1)
    w_sum = np.where(row_keep[None, None, :, None], w.sum(axis=-1, keepdims=True), 1.0)
    w = w / w_sum
    w = np.where(row_keep[None, None, :, None], w, 0.0)
    ctx = np.einsum('bhij,bjhd->bihd', w, V_ext).reshape(B, Sq, Hq * Dh)
    return ctx @ Wo
```

```python
import contextlib
import jax
import jax.numpy as jnp
from jax import lax
from jax.experimental import pallas as pl
from jax.experimental.pallas import tpu as pltpu

F32 = jnp.float32
BF16 = jnp.bfloat16
MESH = pl.DeviceIdType.MESH

N_DEV = 4
B = 2
SQ = 256
ROWS = B * SQ
DM = 512
BLK = 64
QSCALE = 0.125 * 1.4426950408889634
NEG = -1e30
WQ_SUBS = ((0, 32), (32, 96), (128, 128), (256, 256))
NQ_SUB = len(WQ_SUBS)
NO_CHUNK = 4
PERM = (0, 3, 1, 2)
SLOTS = ((0, 0), (0, 1), (3, 0), (1, 1), (3, 1), (1, 0), (2, 0), (2, 1))
L_WO, L_X, L_KV = NQ_SUB, NQ_SUB + 1, NQ_SUB + 3

SCOPES = False


def scope(name):
    return jax.named_scope(name) if SCOPES else contextlib.nullcontext()


def _nt(a, b):
    return lax.dot_general(a, b, (((1,), (1,)), ((), ())), preferred_element_type=F32)


def _nn(a, b):
    return jnp.dot(a, b, preferred_element_type=F32)


def _body(x_hbm, wq_hbm, kt_hbm, vt_hbm, wo_hbm, out_ref,
          x_f32, xb, wq_f32, wo_f32, wq_buf, wo_buf, kt_buf, vt_buf, ctx_buf,
          bdk, bdv,
          ld_sems, send_sem, rq_sems, ro_sems, ready_sem):
    p = lax.axis_index("i")
    left = (p + 3) % N_DEV
    right = (p + 1) % N_DEV
    odd = (p % 2) == 1
    even = jnp.logical_not(odd)

    wq_cps = [pltpu.make_async_copy(wq_hbm.at[pl.ds(r0, n)], wq_f32.at[pl.ds(r0, n)], ld_sems.at[i])
              for i, (r0, n) in enumerate(WQ_SUBS)]
    for c in wq_cps:
        c.start()

    bsem = pltpu.get_barrier_semaphore()

    @pl.when(p != 2)
    def _():
        for nbr in (left, right):
            pl.semaphore_signal(bsem, inc=1, device_id=(nbr,), device_id_type=MESH)

    wo_cp = pltpu.make_async_copy(wo_hbm, wo_f32, ld_sems.at[L_WO])
    wo_cp.start()
    x_cps = [pltpu.make_async_copy(x_hbm.at[pl.ds(b * SQ, SQ)], x_f32.at[pl.ds(b * SQ, SQ)], ld_sems.at[L_X + b])
             for b in range(B)]
    for c in x_cps:
        c.start()
    for s in range(8):
        off, half = SLOTS[s]
        gp = ((p + off) % N_DEV) * 2 + half
        pltpu.make_async_copy(kt_hbm.at[:, gp], kt_buf.at[s], ld_sems.at[L_KV + s // 2]).start()
        pltpu.make_async_copy(vt_hbm.at[:, gp], vt_buf.at[s], ld_sems.at[L_KV + s // 2]).start()

    def rsend(src, dst, rsem, dev):
        pltpu.make_async_remote_copy(src_ref=src, dst_ref=dst, send_sem=send_sem, recv_sem=rsem,
                                     device_id=(dev,), device_id_type=MESH).start()

    def wait_sem(buf, sem):
        pltpu.make_async_copy(buf, buf, sem).wait()

    d1 = jnp.where(p == 1, 1, 0)
    d2 = 1 - d1
    n1 = jnp.where(p == 1, left, right)
    n2 = jnp.where(p == 1, right, left)

    with scope("barrier"):
        pl.semaphore_wait(bsem, jnp.where(odd, 1, 2))

        @pl.when(p == 2)
        def _():
            for nbr in (left, right):
                pl.semaphore_signal(ready_sem, inc=1, device_id=(nbr,), device_id_type=MESH)

    with scope("send_wq"):
        for i, (r0, n) in enumerate(WQ_SUBS):
            rows = pl.ds(r0, n)
            wq_cps[i].wait()
            wq_buf[0, rows, :] = wq_f32[rows, 0:128].astype(BF16)
            wq_buf[1, rows, :] = wq_f32[rows, 128:256].astype(BF16)
            rsend(wq_buf.at[d1, rows], wq_buf.at[2 + d1, rows], rq_sems.at[2 + d1], n1)

            @pl.when(even)
            def _():
                rsend(wq_buf.at[d2, rows], wq_buf.at[2 + d2, rows], rq_sems.at[2 + d2], n2)
        rsend(wq_buf.at[d2], wq_buf.at[4 + d1], rq_sems.at[4 + d1], n1)

    with scope("ready"):
        @pl.when(odd)
        def _():
            pl.semaphore_wait(ready_sem, 1)
            rsend(wq_buf.at[d2], wq_buf.at[2 + d2], rq_sems.at[2 + d2], n2)
        rsend(wq_buf.at[d1], wq_buf.at[4 + d2], rq_sems.at[4 + d2], n2)

    with scope("send_wo"):
        wo_cp.wait()
        wo_buf[0] = wo_f32[0:128, :].astype(BF16)
        wo_buf[1] = wo_f32[128:256, :].astype(BF16)
        rsend(wo_buf.at[0], wo_buf.at[2], ro_sems.at[2], right)
        rsend(wo_buf.at[1], wo_buf.at[3], ro_sems.at[3], left)

    for b in range(B):
        with scope("wait_x"):
            x_cps[b].wait()
        with scope("cast_x"):
            for j, t in enumerate(PERM):
                xb[pl.ds(b * SQ + j * BLK, BLK), :] = x_f32[pl.ds(b * SQ + t * BLK, BLK), :].astype(BF16)

    lo64 = lax.broadcasted_iota(jnp.int32, (BLK, 128), 1) < 64
    lo128 = lax.broadcasted_iota(jnp.int32, (2 * BLK, 128), 1) < 64
    r_ = lax.broadcasted_iota(jnp.int32, (128, 128), 0)
    ones_bd = jnp.where((r_ < 64) == lo128, 1.0, 0.0).astype(BF16)

    x0 = 3 - (p % 3)
    x1 = 3 - ((p + 1) % 3)
    x2 = 3 - ((p + 2) % 3)
    is0 = p == 0

    def build_bd(src, dst):
        for c in range(2):
            col = src[:, c * 128:(c + 1) * 128]
            top, bot = col[0:64], col[64:128]
            rt, rb = pltpu.roll(top, 64, 1), pltpu.roll(bot, 64, 1)
            dst[2 * c, 0:64, :] = jnp.where(lo64, top, 0.0).astype(BF16)
            dst[2 * c, 64:128, :] = jnp.where(lo64, 0.0, rb).astype(BF16)
            dst[2 * c + 1, 0:64, :] = jnp.where(lo64, rt, 0.0).astype(BF16)
            dst[2 * c + 1, 64:128, :] = jnp.where(lo64, 0.0, bot).astype(BF16)

    def seg_max(m):
        m1 = jnp.max(jnp.where(lo128, m, NEG), axis=1, keepdims=True)
        m2 = jnp.max(jnp.where(lo128, NEG, m), axis=1, keepdims=True)
        return jnp.where(lo128, m1, m2)

    def attn_unit(qq, bk, bv):
        qa, qb_ = qq[0:128], qq[128:256]
        s0 = _nn(qq, bk[0])
        sa = _nn(qa, bk[x0])
        s1 = _nn(qb_, bk[x1])
        s2 = _nn(qb_, bk[x2])
        s1 = jnp.concatenate([s1[0:64], jnp.where(is0, s1[64:128], NEG)], axis=0)
        s2 = jnp.concatenate([jnp.where(is0, s2[0:64], NEG), s2[64:128]], axis=0)
        s0a, s0b = s0[0:128], s0[128:256]
        ma = seg_max(jnp.maximum(s0a, sa))
        mb = seg_max(jnp.maximum(jnp.maximum(s0b, s1), s2))
        p0a = jnp.exp2(s0a - ma)
        pa = jnp.exp2(sa - ma)
        p0b = jnp.exp2(s0b - mb)
        p1 = jnp.exp2(s1 - mb)
        p2 = jnp.exp2(s2 - mb)
        p0 = jnp.concatenate([p0a, p0b], axis=0).astype(BF16)
        psum = jnp.concatenate([p0a + pa, p0b + p1 + p2], axis=0).astype(BF16)
        c0 = _nt(p0, bv[0])
        ca = _nt(pa.astype(BF16), bv[x0])
        cb = _nt(p1.astype(BF16), bv[x1]) + _nt(p2.astype(BF16), bv[x2])
        den = _nn(psum, ones_bd)
        return ((c0 + jnp.concatenate([ca, cb], axis=0)) / den).astype(BF16)

    def attn_group(g):
        for h in range(2):
            s = 2 * g + h
            for b in range(B):
                build_bd(kt_buf[s, b], bdk.at[2 * h + b])
                build_bd(vt_buf[s, b], bdv.at[2 * h + b])
        for h in range(2):
            s = 2 * g + h
            q = (_nn(xb[...], wq_buf[s]) * QSCALE).astype(BF16)
            for b in range(B):
                ctx = attn_unit(q[b * SQ:(b + 1) * SQ], bdk.at[2 * h + b], bdv.at[2 * h + b])
                for j, t in enumerate(PERM):
                    ctx_buf[s, pl.ds(b * SQ + t * BLK, BLK), :] = ctx[j * BLK:(j + 1) * BLK]

    cw = DM // NO_CHUNK

    def loop_body(g, carry):
        @pl.when(g == 1)
        def _():
            with scope("p1"):
                wait_sem(wq_buf.at[2], rq_sems.at[2])
                rsend(wq_buf.at[2], wq_buf.at[6], rq_sems.at[6], right)
                rsend(wo_buf.at[1], wo_buf.at[4], ro_sems.at[4], right)
                wait_sem(wq_buf.at[3], rq_sems.at[3])
                rsend(wq_buf.at[3], wq_buf.at[7], rq_sems.at[7], left)
                rsend(wo_buf.at[0], wo_buf.at[5], ro_sems.at[5], left)

        @pl.when(g == 3)
        def _():
            with scope("p2"):
                wait_sem(wo_buf.at[2], ro_sems.at[2])
                for c in range(NO_CHUNK):
                    cols = pl.ds(c * cw, cw)
                    rsend(wo_buf.at[2, :, cols], wo_buf.at[6, :, cols], ro_sems.at[6 + 2 * c], right)
                wait_sem(wo_buf.at[3], ro_sems.at[3])
                for c in range(NO_CHUNK):
                    cols = pl.ds(c * cw, cw)
                    rsend(wo_buf.at[3, :, cols], wo_buf.at[7, :, cols], ro_sems.at[7 + 2 * c], left)
            with scope("oproj1"):
                acc = _nn(ctx_buf[0], wo_buf[0])
                for s in range(1, 4):
                    acc = acc + _nn(ctx_buf[s], wo_buf[s])
                out_ref[...] = acc

        @pl.when(g >= 2)
        def _():
            with scope("wq_wait"):
                wait_sem(wq_buf.at[2 * g], rq_sems.at[2 * g])
                wait_sem(wq_buf.at[2 * g + 1], rq_sems.at[2 * g + 1])

        with scope("kv_wait"):
            wait_sem(kt_buf.at[pl.ds(2 * g, 2)], ld_sems.at[L_KV + g])
            wait_sem(vt_buf.at[pl.ds(2 * g, 2)], ld_sems.at[L_KV + g])
        with scope("attn"):
            attn_group(g)
        return carry

    lax.fori_loop(0, 4, loop_body, 0)

    with scope("w45"):
        wait_sem(wo_buf.at[4], ro_sems.at[4])
        wait_sem(wo_buf.at[5], ro_sems.at[5])
    with scope("oproj2"):
        out_ref[...] += _nn(ctx_buf[4], wo_buf[4]) + _nn(ctx_buf[5], wo_buf[5])
    for c in range(NO_CHUNK):
        cols = pl.ds(c * cw, cw)
        with scope("w67"):
            wait_sem(wo_buf.at[6, :, cols], ro_sems.at[6 + 2 * c])
            wait_sem(wo_buf.at[7, :, cols], ro_sems.at[7 + 2 * c])
        with scope("oproj3"):
            for r in range(2):
                rows = pl.ds(r * 256, 256)
                out_ref[rows, cols] += (_nn(ctx_buf[6, rows, :], wo_buf[6, :, cols])
                                        + _nn(ctx_buf[7, rows, :], wo_buf[7, :, cols]))

    with scope("drain"):
        wait_sem(wq_buf.at[pl.ds(0, 6)], send_sem)
        wait_sem(wo_buf.at[pl.ds(0, 6)], send_sem)


def pallas_dist_sparse_attn_blocksparse_qseq_b2_sq256_skv256_hq4_dh64_kernel(x, Wq, K_ext, V_ext, Wo):
    kt = jnp.transpose(K_ext, (0, 2, 3, 1)).reshape(B, 8, 128, 256)
    vt = jnp.transpose(V_ext, (0, 2, 3, 1)).reshape(B, 8, 128, 256)
    x2 = x.reshape(ROWS, DM)
    out = pl.pallas_call(
        _body,
        out_shape=jax.ShapeDtypeStruct((ROWS, DM), F32),
        in_specs=[pl.BlockSpec(memory_space=pl.ANY)] * 5,
        out_specs=pl.BlockSpec(memory_space=pltpu.VMEM),
        scratch_shapes=[
            pltpu.VMEM((ROWS, DM), F32),
            pltpu.VMEM((ROWS, DM), BF16),
            pltpu.VMEM((DM, 256), F32),
            pltpu.VMEM((256, DM), F32),
            pltpu.VMEM((8, DM, 128), BF16),
            pltpu.VMEM((8, 128, DM), BF16),
            pltpu.VMEM((8, B, 128, 256), F32),
            pltpu.VMEM((8, B, 128, 256), F32),
            pltpu.VMEM((8, ROWS, 128), BF16),
            pltpu.VMEM((4, 4, 128, 128), BF16),
            pltpu.VMEM((4, 4, 128, 128), BF16),
            pltpu.SemaphoreType.DMA((L_KV + 4,)),
            pltpu.SemaphoreType.DMA,
            pltpu.SemaphoreType.DMA((8,)),
            pltpu.SemaphoreType.DMA((6 + 2 * NO_CHUNK,)),
            pltpu.SemaphoreType.REGULAR,
        ],
        compiler_params=pltpu.CompilerParams(
            collective_id=0,
            vmem_limit_bytes=48 * 1024 * 1024,
            disable_semaphore_checks=True,
            disable_bounds_checks=True,
        ),
    )(x2, Wq, kt, vt, Wo)
    return out.reshape(B, SQ, DM)
```

```python
import jax
import jax.numpy as jnp
from jax import lax
from jax.experimental import pallas as pl
from jax.experimental.pallas import tpu as pltpu

F32 = jnp.float32
BF16 = jnp.bfloat16
MESH = pl.DeviceIdType.MESH

B = 2
SQ = 256
ROWS = B * SQ
DM = 512
BLK = 64
QSCALE = 0.125 * 1.4426950408889634
NEG = -1e30

HEAD = 32
WQ_SUBS = ((32, 16), (48, 32), (80, 64), (144, 112), (256, 256), (0, HEAD))
NQ_SUB = len(WQ_SUBS)
NO_CHUNK = 4
CW = DM // NO_CHUNK
PERM = (0, 3, 1, 2)
SLOTS = ((0, 0), (0, 1), (3, 0), (1, 1), (3, 1), (1, 0), (2, 0), (2, 1))
L_WO, L_X, L_KV = NQ_SUB, NQ_SUB + 1, NQ_SUB + 3


def _nt(a, b):
    return lax.dot_general(a, b, (((1,), (1,)), ((), ())), preferred_element_type=F32)


def _nn(a, b):
    return jnp.dot(a, b, preferred_element_type=F32)


def _body(x_hbm, wq_hbm, kt_hbm, vt_hbm, wo_hbm, out_ref,
          x_f32, xb, wq_f32, wo_f32, wq_buf, wo_buf, kv_buf, ctx_buf,
          bdk, bdv, head_buf, wl_buf, cl_buf,
          ld_sems, send_sem, rq_sems, ro_sems, ready_sem):
    wq_cps = [pltpu.make_async_copy(wq_hbm.at[pl.ds(r0, n)], wq_f32.at[pl.ds(r0, n)], ld_sems.at[i])
              for i, (r0, n) in enumerate(WQ_SUBS)]
    wq_cps[0].start()

    p = lax.axis_index("i")
    left = (p + 3) & 3
    right = (p + 1) & 3
    odd = (p & 1) == 1
    even = (p & 1) == 0

    def rsend(src, dst, rsem, dev):
        pltpu.make_async_remote_copy(src_ref=src, dst_ref=dst, send_sem=send_sem, recv_sem=rsem,
                                     device_id=(dev,), device_id_type=MESH).start()

    def wait_sem(buf, sem):
        pltpu.make_async_copy(buf, buf, sem).wait()

    d1 = jnp.where(p == 1, 1, 0)
    d2 = 1 - d1
    n1 = jnp.where(p == 1, left, right)
    n2 = jnp.where(p == 1, right, left)

    def send_head(src, d, n):
        col = pl.multiple_of(d * 128, 128)
        rsend(src.at[pl.ds(0, HEAD), pl.ds(col, 128)], head_buf.at[d], rq_sems.at[d], n)

    bsem = pltpu.get_barrier_semaphore()

    @pl.when(p != 2)
    def _():
        for nbr in (left, right):
            pl.semaphore_signal(bsem, inc=1, device_id=(nbr,), device_id_type=MESH)

    @pl.when(odd)
    def _():
        pl.semaphore_wait(bsem, 1)
        send_head(wq_hbm, d1, n1)

    @pl.when(p == 2)
    def _():
        pl.semaphore_wait(bsem, 2)
        send_head(wq_hbm, d1, n1)
        send_head(wq_hbm, d2, n2)
        for nbr in (left, right):
            pl.semaphore_signal(ready_sem, inc=1, device_id=(nbr,), device_id_type=MESH)

    for c in wq_cps[1:]:
        c.start()
    wo_cp = pltpu.make_async_copy(wo_hbm, wo_f32, ld_sems.at[L_WO])
    wo_cp.start()
    x_cps = [pltpu.make_async_copy(x_hbm.at[pl.ds(b * SQ, SQ)], x_f32.at[pl.ds(b * SQ, SQ)], ld_sems.at[L_X + b])
             for b in range(B)]
    for c in x_cps:
        c.start()
    for s, (off, half) in enumerate(SLOTS):
        gp = ((p + off) & 3) * 2 + half
        pltpu.make_async_copy(kt_hbm.at[:, gp], kv_buf.at[s, 0], ld_sems.at[L_KV + s // 2]).start()
        pltpu.make_async_copy(vt_hbm.at[:, gp], kv_buf.at[s, 1], ld_sems.at[L_KV + s // 2]).start()

    @pl.when(p == 0)
    def _():
        pl.semaphore_wait(bsem, 2)

    for i, (r0, n) in enumerate(WQ_SUBS):
        rows = pl.ds(r0, n)
        wq_cps[i].wait()
        wq_buf[0, rows, :] = wq_f32[rows, 0:128].astype(BF16)
        wq_buf[1, rows, :] = wq_f32[rows, 128:256].astype(BF16)
        if r0 == 0:
            continue
        rsend(wq_buf.at[d1, rows], wq_buf.at[2 + d1, rows], rq_sems.at[2 + d1], n1)

        @pl.when(even)
        def _():
            rsend(wq_buf.at[d2, rows], wq_buf.at[2 + d2, rows], rq_sems.at[2 + d2], n2)

    @pl.when(p == 0)
    def _():
        send_head(wq_f32, d1, n1)
        send_head(wq_f32, d2, n2)
    rsend(wq_buf.at[d2], wq_buf.at[4 + d1], rq_sems.at[4 + d1], n1)

    tail_rows = pl.ds(HEAD, DM - HEAD)
    @pl.when(odd)
    def _():
        pl.semaphore_wait(ready_sem, 1)
        rsend(wq_buf.at[d2, tail_rows], wq_buf.at[2 + d2, tail_rows], rq_sems.at[2 + d2], n2)
        send_head(wq_f32, d2, n2)
    rsend(wq_buf.at[d1], wq_buf.at[4 + d2], rq_sems.at[4 + d2], n2)

    wo_cp.wait()
    wo_buf[0] = wo_f32[0:128, :].astype(BF16)
    wo_buf[1] = wo_f32[128:256, :].astype(BF16)
    rsend(wo_buf.at[0], wo_buf.at[2], ro_sems.at[0], right)
    rsend(wo_buf.at[1], wo_buf.at[3], ro_sems.at[1], left)

    for b in range(B):
        x_cps[b].wait()
        for j, t in enumerate(PERM):
            xb[pl.ds(b * SQ + j * BLK, BLK), :] = x_f32[pl.ds(b * SQ + t * BLK, BLK), :].astype(BF16)

    lo64 = lax.broadcasted_iota(jnp.int32, (BLK, 128), 1) < 64
    lo128 = lax.broadcasted_iota(jnp.int32, (2 * BLK, 128), 1) < 64
    top128 = lax.broadcasted_iota(jnp.int32, (128, 128), 0) < 64
    ones_bd = jnp.where(top128 == lo128, 1.0, 0.0).astype(BF16)

    x0 = 3 - (p % 3)
    x1 = 3 - ((p + 1) % 3)
    x2 = 3 - ((p + 2) % 3)
    is0 = p == 0

    def build_bd(src, dst):
        for c in range(2):
            col = src[:, c * 128:(c + 1) * 128]
            top, bot = col[0:64], col[64:128]
            rt, rb = pltpu.roll(top, 64, 1), pltpu.roll(bot, 64, 1)
            dst[2 * c, 0:64, :] = jnp.where(lo64, top, 0.0).astype(BF16)
            dst[2 * c, 64:128, :] = jnp.where(lo64, 0.0, rb).astype(BF16)
            dst[2 * c + 1, 0:64, :] = jnp.where(lo64, rt, 0.0).astype(BF16)
            dst[2 * c + 1, 64:128, :] = jnp.where(lo64, 0.0, bot).astype(BF16)

    def seg_max(m):
        m1 = jnp.max(jnp.where(lo128, m, NEG), axis=1, keepdims=True)
        m2 = jnp.max(jnp.where(lo128, NEG, m), axis=1, keepdims=True)
        return jnp.where(lo128, m1, m2)

    def attn_unit(qq, bk, bv):
        qa, qb_ = qq[0:128], qq[128:256]
        s0 = _nn(qq, bk[0])
        sa = _nn(qa, bk[x0])
        s1 = _nn(qb_, bk[x1])
        s2 = _nn(qb_, bk[x2])
        s1 = jnp.concatenate([s1[0:64], jnp.where(is0, s1[64:128], NEG)], axis=0)
        s2 = jnp.concatenate([jnp.where(is0, s2[0:64], NEG), s2[64:128]], axis=0)
        s0a, s0b = s0[0:128], s0[128:256]
        ma = seg_max(jnp.maximum(s0a, sa))
        mb = seg_max(jnp.maximum(jnp.maximum(s0b, s1), s2))
        p0a = jnp.exp2(s0a - ma)
        pa = jnp.exp2(sa - ma)
        p0b = jnp.exp2(s0b - mb)
        p1 = jnp.exp2(s1 - mb)
        p2 = jnp.exp2(s2 - mb)
        p0 = jnp.concatenate([p0a, p0b], axis=0).astype(BF16)
        psum = jnp.concatenate([p0a + pa, p0b + p1 + p2], axis=0).astype(BF16)
        c0 = _nt(p0, bv[0])
        ca = _nt(pa.astype(BF16), bv[x0])
        cb = _nt(p1.astype(BF16), bv[x1]) + _nt(p2.astype(BF16), bv[x2])
        den = _nn(psum, ones_bd)
        return ((c0 + jnp.concatenate([ca, cb], axis=0)) / den).astype(BF16)

    def attn_group(g):
        for h in range(2):
            for b in range(B):
                build_bd(kv_buf[2 * g + h, 0, b], bdk.at[2 * h + b])
                build_bd(kv_buf[2 * g + h, 1, b], bdv.at[2 * h + b])
        for h in range(2):
            s = 2 * g + h
            q = (_nn(xb[...], wq_buf[s]) * QSCALE).astype(BF16)
            for b in range(B):
                ctx = attn_unit(q[b * SQ:(b + 1) * SQ], bdk.at[2 * h + b], bdv.at[2 * h + b])
                for j, t in enumerate(PERM):
                    ctx_buf[s, pl.ds(b * SQ + t * BLK, BLK), :] = ctx[j * BLK:(j + 1) * BLK]

    lcols = pl.ds((NO_CHUNK - 1) * CW, CW)

    def loop_body(g, carry):
        @pl.when(g == 1)
        def _():
            for d, nbr in ((0, right), (1, left)):
                wait_sem(head_buf.at[d], rq_sems.at[d])
                wq_buf[2 + d, pl.ds(0, HEAD), :] = head_buf[d].astype(BF16)
                wait_sem(wq_buf.at[2 + d, tail_rows], rq_sems.at[2 + d])
                rsend(wq_buf.at[2 + d], wq_buf.at[6 + d], rq_sems.at[6 + d], nbr)
                rsend(wo_buf.at[1 - d], wo_buf.at[4 + d], ro_sems.at[2 + d], nbr)

        @pl.when(g == 3)
        def _():
            for d, nbr in ((0, right), (1, left)):
                wait_sem(wo_buf.at[2 + d], ro_sems.at[d])
                for c in range(NO_CHUNK - 1):
                    cols = pl.ds(c * CW, CW)
                    rsend(wo_buf.at[2 + d, :, cols], wo_buf.at[6 + d, :, cols], ro_sems.at[4 + 2 * c + d], nbr)
                for j in range(2):
                    half = pl.ds(64 * ((d + j) % 2), 64)
                    rsend(wo_buf.at[2 + d, half, lcols], wl_buf.at[j, half],
                          ro_sems.at[4 + 2 * (NO_CHUNK - 1 + j) + d], nbr)
            acc = _nn(ctx_buf[0], wo_buf[0])
            for s in range(1, 4):
                acc = acc + _nn(ctx_buf[s], wo_buf[s])
            out_ref[...] = acc

        @pl.when(g >= 2)
        def _():
            wait_sem(wq_buf.at[2 * g], rq_sems.at[2 * g])
            wait_sem(wq_buf.at[2 * g + 1], rq_sems.at[2 * g + 1])

        wait_sem(kv_buf.at[pl.ds(2 * g, 2)], ld_sems.at[L_KV + g])
        attn_group(g)
        return carry

    lax.fori_loop(0, 4, loop_body, 0)

    lo_u = lax.broadcasted_iota(jnp.int32, (ROWS // 2, 128), 1) < 64
    c6 = pltpu.bitcast(ctx_buf[6], jnp.uint32)
    c7 = pltpu.bitcast(ctx_buf[7], jnp.uint32)
    cl_buf[0] = pltpu.bitcast(jnp.where(lo_u, c6, c7), BF16)
    cl_buf[1] = pltpu.bitcast(jnp.where(lo_u, c7, c6), BF16)
    wait_sem(wo_buf.at[4], ro_sems.at[2])
    wait_sem(wo_buf.at[5], ro_sems.at[3])
    out_ref[...] += _nn(ctx_buf[4], wo_buf[4]) + _nn(ctx_buf[5], wo_buf[5])
    for c in range(NO_CHUNK - 1):
        cols = pl.ds(c * CW, CW)
        wait_sem(wo_buf.at[6, :, cols], ro_sems.at[4 + 2 * c])
        wait_sem(wo_buf.at[7, :, cols], ro_sems.at[5 + 2 * c])
        for r in range(2):
            rows = pl.ds(r * 256, 256)
            out_ref[rows, cols] += (_nn(ctx_buf[6, rows, :], wo_buf[6, :, cols])
                                    + _nn(ctx_buf[7, rows, :], wo_buf[7, :, cols]))
    for j in range(2):
        for d in range(2):
            half = pl.ds(64 * ((d + j) % 2), 64)
            wait_sem(wl_buf.at[j, half], ro_sems.at[4 + 2 * (NO_CHUNK - 1 + j) + d])
        for r in range(4):
            rows = pl.ds(r * 128, 128)
            out_ref[rows, lcols] += _nn(cl_buf[j, rows, :], wl_buf[j])

    wait_sem(head_buf, send_sem)
    wait_sem(wq_buf.at[pl.ds(0, 2), tail_rows], send_sem)
    wait_sem(wq_buf.at[pl.ds(0, 4)], send_sem)
    wait_sem(wo_buf.at[pl.ds(0, 6)], send_sem)


def _compiler_params():
    kw = dict(collective_id=0, vmem_limit_bytes=48 * 1024 * 1024)
    for name in ("disable_semaphore_checks", "disable_bounds_checks"):
        if hasattr(pltpu.CompilerParams, name):
            kw[name] = True
    return pltpu.CompilerParams(**kw)


def pallas_dist_sparse_attn_blocksparse_qseq_b2_sq256_skv256_hq4_dh64_kernel(x, Wq, K_ext, V_ext, Wo):
    kt = jnp.transpose(K_ext, (0, 2, 3, 1)).reshape(B, 8, 128, 256)
    vt = jnp.transpose(V_ext, (0, 2, 3, 1)).reshape(B, 8, 128, 256)
    out = pl.pallas_call(
        _body,
        out_shape=jax.ShapeDtypeStruct((ROWS, DM), F32),
        in_specs=[pl.BlockSpec(memory_space=pl.ANY)] * 5,
        out_specs=pl.BlockSpec(memory_space=pltpu.VMEM),
        scratch_shapes=[
            pltpu.VMEM((ROWS, DM), F32),
            pltpu.VMEM((ROWS, DM), BF16),
            pltpu.VMEM((DM, 256), F32),
            pltpu.VMEM((256, DM), F32),
            pltpu.VMEM((8, DM, 128), BF16),
            pltpu.VMEM((8, 128, DM), BF16),
            pltpu.VMEM((8, 2, B, 128, 256), F32),
            pltpu.VMEM((8, ROWS, 128), BF16),
            pltpu.VMEM((4, 4, 128, 128), BF16),
            pltpu.VMEM((4, 4, 128, 128), BF16),
            pltpu.VMEM((2, HEAD, 128), F32),
            pltpu.VMEM((2, 128, 128), BF16),
            pltpu.VMEM((2, ROWS, 128), BF16),
            pltpu.SemaphoreType.DMA((L_KV + 4,)),
            pltpu.SemaphoreType.DMA,
            pltpu.SemaphoreType.DMA((8,)),
            pltpu.SemaphoreType.DMA((6 + 2 * NO_CHUNK,)),
            pltpu.SemaphoreType.REGULAR,
        ],
        compiler_params=_compiler_params(),
    )(x.reshape(ROWS, DM), Wq, kt, vt, Wo)
    return out.reshape(B, SQ, DM)
```

```python
import jax
import jax.numpy as jnp
from jax import lax
from jax.experimental import pallas as pl
from jax.experimental.pallas import tpu as pltpu

F32 = jnp.float32
BF16 = jnp.bfloat16
MESH = pl.DeviceIdType.MESH

B = 2
SQ = 256
ROWS = B * SQ
DM = 512
BLK = 64
QSCALE = 0.125 * 1.4426950408889634
NEG = -1e30

HEAD = 32
WQ_SUBS = ((32, 16), (48, 32), (80, 64), (144, 112), (256, 256), (0, HEAD))
NQ_SUB = len(WQ_SUBS)
NO_CHUNK = 4
CW = DM // NO_CHUNK
PERM = (0, 3, 1, 2)
SLOTS = ((0, 0), (0, 1), (3, 0), (1, 1), (3, 1), (1, 0), (2, 0), (2, 1))
L_WO, L_X, L_KV = NQ_SUB, NQ_SUB + 1, NQ_SUB + 3
S_HEAD, S_WQ1, S_WQ, S_WO = range(4)


def _nt(a, b):
    return lax.dot_general(a, b, (((1,), (1,)), ((), ())), preferred_element_type=F32)


def _nn(a, b):
    return jnp.dot(a, b, preferred_element_type=F32)


def _body(x_hbm, wq_hbm, kt_hbm, vt_hbm, wo_hbm, out_ref,
          x_f32, xb, wq_f32, wo_f32, wq_buf, wo_buf, kv_buf, ctx_buf,
          bdk, bdv, head_buf, wl_buf, cl_buf,
          ld_sems, send_sems, rq_sems, ro_sems, ready_sem):
    wq_cps = [pltpu.make_async_copy(wq_hbm.at[pl.ds(r0, n)], wq_f32.at[pl.ds(r0, n)], ld_sems.at[i])
              for i, (r0, n) in enumerate(WQ_SUBS)]
    wq_cps[0].start()

    p = lax.axis_index("i")
    left = (p + 3) & 3
    right = (p + 1) & 3
    odd = (p & 1) == 1
    even = (p & 1) == 0

    def rsend(kind, src, dst, rsem, dev):
        pltpu.make_async_remote_copy(src_ref=src, dst_ref=dst, send_sem=send_sems.at[kind], recv_sem=rsem,
                                     device_id=(dev,), device_id_type=MESH).start()

    def wait_sem(buf, sem):
        pltpu.make_async_copy(buf, buf, sem).wait()

    d1 = jnp.where(p == 1, 1, 0)
    d2 = 1 - d1
    n1 = jnp.where(p == 1, left, right)
    n2 = jnp.where(p == 1, right, left)

    def send_head(src, d, n):
        col = pl.multiple_of(d * 128, 128)
        rsend(S_HEAD, src.at[pl.ds(0, HEAD), pl.ds(col, 128)], head_buf.at[d], rq_sems.at[d], n)

    bsem = pltpu.get_barrier_semaphore()

    @pl.when(p != 2)
    def _():
        for nbr in (left, right):
            pl.semaphore_signal(bsem, inc=1, device_id=(nbr,), device_id_type=MESH)

    @pl.when(odd)
    def _():
        pl.semaphore_wait(bsem, 1)
        send_head(wq_hbm, d1, n1)

    @pl.when(p == 2)
    def _():
        pl.semaphore_wait(bsem, 2)
        send_head(wq_hbm, d1, n1)
        send_head(wq_hbm, d2, n2)
        for nbr in (left, right):
            pl.semaphore_signal(ready_sem, inc=1, device_id=(nbr,), device_id_type=MESH)

    for c in wq_cps[1:]:
        c.start()
    wo_cp = pltpu.make_async_copy(wo_hbm, wo_f32, ld_sems.at[L_WO])
    wo_cp.start()
    x_cps = [pltpu.make_async_copy(x_hbm.at[pl.ds(b * SQ, SQ)], x_f32.at[pl.ds(b * SQ, SQ)], ld_sems.at[L_X + b])
             for b in range(B)]
    for c in x_cps:
        c.start()
    for s, (off, half) in enumerate(SLOTS):
        gp = ((p + off) & 3) * 2 + half
        pltpu.make_async_copy(kt_hbm.at[:, gp], kv_buf.at[s, 0], ld_sems.at[L_KV + s // 2]).start()
        pltpu.make_async_copy(vt_hbm.at[:, gp], kv_buf.at[s, 1], ld_sems.at[L_KV + s // 2]).start()

    @pl.when(p == 0)
    def _():
        pl.semaphore_wait(bsem, 2)

    for i, (r0, n) in enumerate(WQ_SUBS):
        rows = pl.ds(r0, n)
        wq_cps[i].wait()
        wq_buf[0, rows, :] = wq_f32[rows, 0:128].astype(BF16)
        wq_buf[1, rows, :] = wq_f32[rows, 128:256].astype(BF16)
        if r0 == 0:
            continue
        rsend(S_WQ1, wq_buf.at[d1, rows], wq_buf.at[2 + d1, rows], rq_sems.at[2 + d1], n1)

        @pl.when(even)
        def _():
            rsend(S_WQ1, wq_buf.at[d2, rows], wq_buf.at[2 + d2, rows], rq_sems.at[2 + d2], n2)

    @pl.when(p == 0)
    def _():
        send_head(wq_f32, d1, n1)
        send_head(wq_f32, d2, n2)
    rsend(S_WQ, wq_buf.at[d2], wq_buf.at[4 + d1], rq_sems.at[4 + d1], n1)

    tail_rows = pl.ds(HEAD, DM - HEAD)
    @pl.when(odd)
    def _():
        pl.semaphore_wait(ready_sem, 1)
        rsend(S_WQ1, wq_buf.at[d2, tail_rows], wq_buf.at[2 + d2, tail_rows], rq_sems.at[2 + d2], n2)
        send_head(wq_f32, d2, n2)
    rsend(S_WQ, wq_buf.at[d1], wq_buf.at[4 + d2], rq_sems.at[4 + d2], n2)

    wo_cp.wait()
    wo_buf[0] = wo_f32[0:128, :].astype(BF16)
    wo_buf[1] = wo_f32[128:256, :].astype(BF16)
    rsend(S_WO, wo_buf.at[0], wo_buf.at[2], ro_sems.at[0], right)
    rsend(S_WO, wo_buf.at[1], wo_buf.at[3], ro_sems.at[1], left)

    for b in range(B):
        x_cps[b].wait()
        for j, t in enumerate(PERM):
            xb[pl.ds(b * SQ + j * BLK, BLK), :] = x_f32[pl.ds(b * SQ + t * BLK, BLK), :].astype(BF16)

    lo64 = lax.broadcasted_iota(jnp.int32, (BLK, 128), 1) < 64
    lo128 = lax.broadcasted_iota(jnp.int32, (2 * BLK, 128), 1) < 64
    top128 = lax.broadcasted_iota(jnp.int32, (128, 128), 0) < 64
    ones_bd = jnp.where(top128 == lo128, 1.0, 0.0).astype(BF16)

    x0 = 3 - (p % 3)
    x1 = 3 - ((p + 1) % 3)
    x2 = 3 - ((p + 2) % 3)
    is0 = p == 0

    def build_bd(src, dst):
        for c in range(2):
            col = src[:, c * 128:(c + 1) * 128]
            top, bot = col[0:64], col[64:128]
            rt, rb = pltpu.roll(top, 64, 1), pltpu.roll(bot, 64, 1)
            dst[2 * c, 0:64, :] = jnp.where(lo64, top, 0.0).astype(BF16)
            dst[2 * c, 64:128, :] = jnp.where(lo64, 0.0, rb).astype(BF16)
            dst[2 * c + 1, 0:64, :] = jnp.where(lo64, rt, 0.0).astype(BF16)
            dst[2 * c + 1, 64:128, :] = jnp.where(lo64, 0.0, bot).astype(BF16)

    def seg_max(m):
        m1 = jnp.max(jnp.where(lo128, m, NEG), axis=1, keepdims=True)
        m2 = jnp.max(jnp.where(lo128, NEG, m), axis=1, keepdims=True)
        return jnp.where(lo128, m1, m2)

    def attn_unit(qq, bk, bv):
        qa, qb_ = qq[0:128], qq[128:256]
        s0 = _nn(qq, bk[0])
        sa = _nn(qa, bk[x0])
        s1 = _nn(qb_, bk[x1])
        s2 = _nn(qb_, bk[x2])
        s1 = jnp.concatenate([s1[0:64], jnp.where(is0, s1[64:128], NEG)], axis=0)
        s2 = jnp.concatenate([jnp.where(is0, s2[0:64], NEG), s2[64:128]], axis=0)
        s0a, s0b = s0[0:128], s0[128:256]
        ma = seg_max(jnp.maximum(s0a, sa))
        mb = seg_max(jnp.maximum(jnp.maximum(s0b, s1), s2))
        p0a = jnp.exp2(s0a - ma)
        pa = jnp.exp2(sa - ma)
        p0b = jnp.exp2(s0b - mb)
        p1 = jnp.exp2(s1 - mb)
        p2 = jnp.exp2(s2 - mb)
        p0 = jnp.concatenate([p0a, p0b], axis=0).astype(BF16)
        psum = jnp.concatenate([p0a + pa, p0b + p1 + p2], axis=0).astype(BF16)
        c0 = _nt(p0, bv[0])
        ca = _nt(pa.astype(BF16), bv[x0])
        cb = _nt(p1.astype(BF16), bv[x1]) + _nt(p2.astype(BF16), bv[x2])
        den = _nn(psum, ones_bd)
        return ((c0 + jnp.concatenate([ca, cb], axis=0)) / den).astype(BF16)

    def attn_group(g):
        for h in range(2):
            for b in range(B):
                build_bd(kv_buf[2 * g + h, 0, b], bdk.at[2 * h + b])
                build_bd(kv_buf[2 * g + h, 1, b], bdv.at[2 * h + b])
        for h in range(2):
            s = 2 * g + h
            q = (_nn(xb[...], wq_buf[s]) * QSCALE).astype(BF16)
            for b in range(B):
                ctx = attn_unit(q[b * SQ:(b + 1) * SQ], bdk.at[2 * h + b], bdv.at[2 * h + b])
                for j, t in enumerate(PERM):
                    ctx_buf[s, pl.ds(b * SQ + t * BLK, BLK), :] = ctx[j * BLK:(j + 1) * BLK]

    lcols = pl.ds((NO_CHUNK - 1) * CW, CW)

    def loop_body(g, carry):
        @pl.when(g == 1)
        def _():
            for d, nbr in ((0, right), (1, left)):
                wait_sem(head_buf.at[d], rq_sems.at[d])
                wq_buf[2 + d, pl.ds(0, HEAD), :] = head_buf[d].astype(BF16)
                wait_sem(wq_buf.at[2 + d, tail_rows], rq_sems.at[2 + d])
                rsend(S_WQ, wq_buf.at[2 + d], wq_buf.at[6 + d], rq_sems.at[6 + d], nbr)
                rsend(S_WO, wo_buf.at[1 - d], wo_buf.at[4 + d], ro_sems.at[2 + d], nbr)

        @pl.when(g == 3)
        def _():
            for d, nbr in ((0, right), (1, left)):
                wait_sem(wo_buf.at[2 + d], ro_sems.at[d])
                for c in range(NO_CHUNK - 1):
                    cols = pl.ds(c * CW, CW)
                    rsend(S_WO, wo_buf.at[2 + d, :, cols], wo_buf.at[6 + d, :, cols],
                          ro_sems.at[4 + 2 * c + d], nbr)
                for j in range(2):
                    half = pl.ds(64 * ((d + j) % 2), 64)
                    rsend(S_WO, wo_buf.at[2 + d, half, lcols], wl_buf.at[j, half],
                          ro_sems.at[4 + 2 * (NO_CHUNK - 1 + j) + d], nbr)
            acc = _nn(ctx_buf[0], wo_buf[0])
            for s in range(1, 4):
                acc = acc + _nn(ctx_buf[s], wo_buf[s])
            out_ref[...] = acc

        @pl.when(g >= 2)
        def _():
            wait_sem(wq_buf.at[2 * g], rq_sems.at[2 * g])
            wait_sem(wq_buf.at[2 * g + 1], rq_sems.at[2 * g + 1])

        wait_sem(kv_buf.at[pl.ds(2 * g, 2)], ld_sems.at[L_KV + g])
        attn_group(g)
        return carry

    lax.fori_loop(0, 4, loop_body, 0)

    lo_u = lax.broadcasted_iota(jnp.int32, (ROWS // 2, 128), 1) < 64
    c6 = pltpu.bitcast(ctx_buf[6], jnp.uint32)
    c7 = pltpu.bitcast(ctx_buf[7], jnp.uint32)
    cl_buf[0] = pltpu.bitcast(jnp.where(lo_u, c6, c7), BF16)
    cl_buf[1] = pltpu.bitcast(jnp.where(lo_u, c7, c6), BF16)
    wait_sem(head_buf, send_sems.at[S_HEAD])
    wait_sem(wq_buf.at[pl.ds(0, 2), tail_rows], send_sems.at[S_WQ1])
    wait_sem(wq_buf.at[pl.ds(0, 4)], send_sems.at[S_WQ])
    wait_sem(wo_buf.at[4], ro_sems.at[2])
    wait_sem(wo_buf.at[5], ro_sems.at[3])
    out_ref[...] += _nn(ctx_buf[4], wo_buf[4]) + _nn(ctx_buf[5], wo_buf[5])
    for c in range(NO_CHUNK - 1):
        cols = pl.ds(c * CW, CW)
        wait_sem(wo_buf.at[6, :, cols], ro_sems.at[4 + 2 * c])
        wait_sem(wo_buf.at[7, :, cols], ro_sems.at[5 + 2 * c])
        for r in range(2):
            rows = pl.ds(r * 256, 256)
            out_ref[rows, cols] += (_nn(ctx_buf[6, rows, :], wo_buf[6, :, cols])
                                    + _nn(ctx_buf[7, rows, :], wo_buf[7, :, cols]))
    for j in range(2):
        for d in range(2):
            half = pl.ds(64 * ((d + j) % 2), 64)
            wait_sem(wl_buf.at[j, half], ro_sems.at[4 + 2 * (NO_CHUNK - 1 + j) + d])
        for r in range(4):
            rows = pl.ds(r * 128, 128)
            out_ref[rows, lcols] += _nn(cl_buf[j, rows, :], wl_buf[j])

    wait_sem(wo_buf.at[pl.ds(0, 6)], send_sems.at[S_WO])


def _compiler_params():
    kw = dict(collective_id=0, vmem_limit_bytes=48 * 1024 * 1024)
    for name in ("disable_semaphore_checks", "disable_bounds_checks"):
        if hasattr(pltpu.CompilerParams, name):
            kw[name] = True
    return pltpu.CompilerParams(**kw)


def pallas_dist_sparse_attn_blocksparse_qseq_b2_sq256_skv256_hq4_dh64_kernel(x, Wq, K_ext, V_ext, Wo):
    kt = jnp.transpose(K_ext, (0, 2, 3, 1)).reshape(B, 8, 128, 256)
    vt = jnp.transpose(V_ext, (0, 2, 3, 1)).reshape(B, 8, 128, 256)
    out = pl.pallas_call(
        _body,
        out_shape=jax.ShapeDtypeStruct((ROWS, DM), F32),
        in_specs=[pl.BlockSpec(memory_space=pl.ANY)] * 5,
        out_specs=pl.BlockSpec(memory_space=pltpu.VMEM),
        scratch_shapes=[
            pltpu.VMEM((ROWS, DM), F32),
            pltpu.VMEM((ROWS, DM), BF16),
            pltpu.VMEM((DM, 256), F32),
            pltpu.VMEM((256, DM), F32),
            pltpu.VMEM((8, DM, 128), BF16),
            pltpu.VMEM((8, 128, DM), BF16),
            pltpu.VMEM((8, 2, B, 128, 256), F32),
            pltpu.VMEM((8, ROWS, 128), BF16),
            pltpu.VMEM((4, 4, 128, 128), BF16),
            pltpu.VMEM((4, 4, 128, 128), BF16),
            pltpu.VMEM((2, HEAD, 128), F32),
            pltpu.VMEM((2, 128, 128), BF16),
            pltpu.VMEM((2, ROWS, 128), BF16),
            pltpu.SemaphoreType.DMA((L_KV + 4,)),
            pltpu.SemaphoreType.DMA((4,)),
            pltpu.SemaphoreType.DMA((8,)),
            pltpu.SemaphoreType.DMA((6 + 2 * NO_CHUNK,)),
            pltpu.SemaphoreType.REGULAR,
        ],
        compiler_params=_compiler_params(),
    )(x.reshape(ROWS, DM), Wq, kt, vt, Wo)
    return out.reshape(B, SQ, DM)
```

```python
import jax
import jax.numpy as jnp
from jax import lax
from jax.experimental import pallas as pl
from jax.experimental.pallas import tpu as pltpu

F32 = jnp.float32
BF16 = jnp.bfloat16
MESH = pl.DeviceIdType.MESH

B = 2
SQ = 256
ROWS = B * SQ
DM = 512
BLK = 64
LOG2E = 1.4426950408889634
QSCALE = 0.125 * LOG2E
MASKED = -1e9 * LOG2E

HEAD = 32
WQ_SUBS = ((32, 16), (48, 32), (80, 64), (144, 112), (256, 256), (0, HEAD))
NQ_SUB = len(WQ_SUBS)
NO_CHUNK = 4
CW = DM // NO_CHUNK
PERM = (0, 3, 1, 2)
SLOTS = ((0, 0), (0, 1), (3, 0), (1, 1), (3, 1), (1, 0), (2, 0), (2, 1))
L_WO, L_X, L_KV = NQ_SUB, NQ_SUB + 1, NQ_SUB + 3
S_HEAD, S_WQ1, S_WQ, S_WO = range(4)


def _nt(a, b):
    return lax.dot_general(a, b, (((1,), (1,)), ((), ())), preferred_element_type=F32)


def _nn(a, b):
    return jnp.dot(a, b, preferred_element_type=F32)


def _body(x_hbm, wq_hbm, kt_hbm, vt_hbm, wo_hbm, out_ref,
          x_f32, xb, wq_f32, wo_f32, wq_buf, wo_buf, kv_buf, ctx_buf,
          bdk, bdv, head_buf, wl_buf, cl_buf,
          ld_sems, send_sems, rq_sems, ro_sems, ready_sem):
    wq_cps = [pltpu.make_async_copy(wq_hbm.at[pl.ds(r0, n)], wq_f32.at[pl.ds(r0, n)], ld_sems.at[i])
              for i, (r0, n) in enumerate(WQ_SUBS)]
    wq_cps[0].start()

    p = lax.axis_index("i")
    left = (p + 3) & 3
    right = (p + 1) & 3
    odd = (p & 1) == 1
    even = (p & 1) == 0

    def rsend(kind, src, dst, rsem, dev):
        pltpu.make_async_remote_copy(src_ref=src, dst_ref=dst, send_sem=send_sems.at[kind], recv_sem=rsem,
                                     device_id=(dev,), device_id_type=MESH).start()

    def wait_sem(buf, sem):
        pltpu.make_async_copy(buf, buf, sem).wait()

    d1 = jnp.where(p == 1, 1, 0)
    d2 = 1 - d1
    n1 = jnp.where(p == 1, left, right)
    n2 = jnp.where(p == 1, right, left)

    def send_head(src, d, n):
        col = pl.multiple_of(d * 128, 128)
        rsend(S_HEAD, src.at[pl.ds(0, HEAD), pl.ds(col, 128)], head_buf.at[d], rq_sems.at[d], n)

    bsem = pltpu.get_barrier_semaphore()

    @pl.when(p != 2)
    def _():
        for nbr in (left, right):
            pl.semaphore_signal(bsem, inc=1, device_id=(nbr,), device_id_type=MESH)

    @pl.when(odd)
    def _():
        pl.semaphore_wait(bsem, 1)
        send_head(wq_hbm, d1, n1)

    @pl.when(p == 2)
    def _():
        pl.semaphore_wait(bsem, 2)
        send_head(wq_hbm, d1, n1)
        send_head(wq_hbm, d2, n2)
        for nbr in (left, right):
            pl.semaphore_signal(ready_sem, inc=1, device_id=(nbr,), device_id_type=MESH)

    for c in wq_cps[1:]:
        c.start()
    wo_cp = pltpu.make_async_copy(wo_hbm, wo_f32, ld_sems.at[L_WO])
    wo_cp.start()
    x_cps = [pltpu.make_async_copy(x_hbm.at[pl.ds(b * SQ, SQ)], x_f32.at[pl.ds(b * SQ, SQ)], ld_sems.at[L_X + b])
             for b in range(B)]
    for c in x_cps:
        c.start()
    for s, (off, half) in enumerate(SLOTS):
        gp = ((p + off) & 3) * 2 + half
        pltpu.make_async_copy(kt_hbm.at[:, gp], kv_buf.at[s, 0], ld_sems.at[L_KV + s // 2]).start()
        pltpu.make_async_copy(vt_hbm.at[:, gp], kv_buf.at[s, 1], ld_sems.at[L_KV + s // 2]).start()

    @pl.when(p == 0)
    def _():
        pl.semaphore_wait(bsem, 2)

    for i, (r0, n) in enumerate(WQ_SUBS):
        rows = pl.ds(r0, n)
        wq_cps[i].wait()
        wq_buf[0, rows, :] = wq_f32[rows, 0:128].astype(BF16)
        wq_buf[1, rows, :] = wq_f32[rows, 128:256].astype(BF16)
        if r0 == 0:
            continue
        rsend(S_WQ1, wq_buf.at[d1, rows], wq_buf.at[2 + d1, rows], rq_sems.at[2 + d1], n1)

        @pl.when(even)
        def _():
            rsend(S_WQ1, wq_buf.at[d2, rows], wq_buf.at[2 + d2, rows], rq_sems.at[2 + d2], n2)

    @pl.when(p == 0)
    def _():
        send_head(wq_f32, d1, n1)
        send_head(wq_f32, d2, n2)
    rsend(S_WQ, wq_buf.at[d2], wq_buf.at[4 + d1], rq_sems.at[4 + d1], n1)

    tail_rows = pl.ds(HEAD, DM - HEAD)
    @pl.when(odd)
    def _():
        pl.semaphore_wait(ready_sem, 1)
        rsend(S_WQ1, wq_buf.at[d2, tail_rows], wq_buf.at[2 + d2, tail_rows], rq_sems.at[2 + d2], n2)
        send_head(wq_f32, d2, n2)
    rsend(S_WQ, wq_buf.at[d1], wq_buf.at[4 + d2], rq_sems.at[4 + d2], n2)

    wo_cp.wait()
    wo_buf[0] = wo_f32[0:128, :].astype(BF16)
    wo_buf[1] = wo_f32[128:256, :].astype(BF16)
    rsend(S_WO, wo_buf.at[0], wo_buf.at[2], ro_sems.at[0], right)
    rsend(S_WO, wo_buf.at[1], wo_buf.at[3], ro_sems.at[1], left)

    for b in range(B):
        x_cps[b].wait()
        for j, t in enumerate(PERM):
            xb[pl.ds(b * SQ + j * BLK, BLK), :] = x_f32[pl.ds(b * SQ + t * BLK, BLK), :].astype(BF16)

    lo64 = lax.broadcasted_iota(jnp.int32, (BLK, 128), 1) < 64
    lo128 = lax.broadcasted_iota(jnp.int32, (2 * BLK, 128), 1) < 64
    top128 = lax.broadcasted_iota(jnp.int32, (128, 128), 0) < 64
    ones_bd = jnp.where(top128 == lo128, 1.0, 0.0).astype(BF16)

    x0 = 3 - (p % 3)
    x1 = 3 - ((p + 1) % 3)
    x2 = 3 - ((p + 2) % 3)
    is0 = p == 0

    def build_bd(src, dst):
        for c in range(2):
            col = src[:, c * 128:(c + 1) * 128]
            top, bot = col[0:64], col[64:128]
            rt, rb = pltpu.roll(top, 64, 1), pltpu.roll(bot, 64, 1)
            dst[2 * c, 0:64, :] = jnp.where(lo64, top, 0.0).astype(BF16)
            dst[2 * c, 64:128, :] = jnp.where(lo64, 0.0, rb).astype(BF16)
            dst[2 * c + 1, 0:64, :] = jnp.where(lo64, rt, 0.0).astype(BF16)
            dst[2 * c + 1, 64:128, :] = jnp.where(lo64, 0.0, bot).astype(BF16)

    def seg_max(m):
        m1 = jnp.max(jnp.where(lo128, m, MASKED), axis=1, keepdims=True)
        m2 = jnp.max(jnp.where(lo128, MASKED, m), axis=1, keepdims=True)
        return jnp.where(lo128, m1, m2)

    ones_rows = jnp.ones((16, 128), BF16)

    def attn_unit(qq, bk, bv):
        qa, qb_ = qq[0:128], qq[128:256]
        s0 = _nn(qq, bk[0])
        sa = _nn(qa, bk[x0])
        s1 = _nn(qb_, bk[x1])
        s2 = _nn(qb_, bk[x2])
        s1 = jnp.concatenate([s1[0:64], jnp.where(is0, s1[64:128], MASKED)], axis=0)
        s2 = jnp.concatenate([jnp.where(is0, s2[0:64], MASKED), s2[64:128]], axis=0)
        s0a, s0b = s0[0:128], s0[128:256]
        ma = seg_max(jnp.maximum(s0a, sa))
        mb = seg_max(jnp.maximum(jnp.maximum(s0b, s1), s2))
        p0a = jnp.exp2(s0a - ma)
        pa = jnp.exp2(sa - ma)
        p0b = jnp.exp2(s0b - mb)
        p1 = jnp.exp2(s1 - mb)
        p2 = jnp.exp2(s2 - mb)
        p0 = jnp.concatenate([p0a, p0b], axis=0).astype(BF16)
        psum = jnp.concatenate([p0a + pa, p0b + p1 + p2], axis=0).astype(BF16)
        ea = jnp.exp2(MASKED - ma)
        eb = jnp.exp2(MASKED - mb)
        c0 = _nt(p0, bv[0])
        ca = _nt(jnp.concatenate([pa.astype(BF16), ones_rows], axis=0), bv[x0])
        cb = (_nt(jnp.concatenate([p1.astype(BF16), ones_rows], axis=0), bv[x1])
              + _nt(jnp.concatenate([p2.astype(BF16), ones_rows], axis=0), bv[x2]))
        ca, cb = ca[0:128] + ea * cb[128:129], cb[0:128] + eb * ca[128:129]
        den = _nn(psum, ones_bd) + jnp.concatenate([ea * (2.0 * BLK), eb * (1.0 * BLK)], axis=0)
        return ((c0 + jnp.concatenate([ca, cb], axis=0)) / den).astype(BF16)

    def attn_group(g):
        for h in range(2):
            for b in range(B):
                build_bd(kv_buf[2 * g + h, 0, b], bdk.at[2 * h + b])
                build_bd(kv_buf[2 * g + h, 1, b], bdv.at[2 * h + b])
        for h in range(2):
            s = 2 * g + h
            q = (_nn(xb[...], wq_buf[s]) * QSCALE).astype(BF16)
            for b in range(B):
                ctx = attn_unit(q[b * SQ:(b + 1) * SQ], bdk.at[2 * h + b], bdv.at[2 * h + b])
                for j, t in enumerate(PERM):
                    ctx_buf[s, pl.ds(b * SQ + t * BLK, BLK), :] = ctx[j * BLK:(j + 1) * BLK]

    lcols = pl.ds((NO_CHUNK - 1) * CW, CW)

    def loop_body(g, carry):
        @pl.when(g == 1)
        def _():
            for d, nbr in ((0, right), (1, left)):
                wait_sem(head_buf.at[d], rq_sems.at[d])
                wq_buf[2 + d, pl.ds(0, HEAD), :] = head_buf[d].astype(BF16)
                wait_sem(wq_buf.at[2 + d, tail_rows], rq_sems.at[2 + d])
                rsend(S_WQ, wq_buf.at[2 + d], wq_buf.at[6 + d], rq_sems.at[6 + d], nbr)
                rsend(S_WO, wo_buf.at[1 - d], wo_buf.at[4 + d], ro_sems.at[2 + d], nbr)

        @pl.when(g == 3)
        def _():
            for d, nbr in ((0, right), (1, left)):
                wait_sem(wo_buf.at[2 + d], ro_sems.at[d])
                for c in range(NO_CHUNK - 1):
                    cols = pl.ds(c * CW, CW)
                    rsend(S_WO, wo_buf.at[2 + d, :, cols], wo_buf.at[6 + d, :, cols],
                          ro_sems.at[4 + 2 * c + d], nbr)
                for j in range(2):
                    half = pl.ds(64 * ((d + j) % 2), 64)
                    rsend(S_WO, wo_buf.at[2 + d, half, lcols], wl_buf.at[j, half],
                          ro_sems.at[4 + 2 * (NO_CHUNK - 1 + j) + d], nbr)
            acc = _nn(ctx_buf[0], wo_buf[0])
            for s in range(1, 4):
                acc = acc + _nn(ctx_buf[s], wo_buf[s])
            out_ref[...] = acc

        @pl.when(g >= 2)
        def _():
            wait_sem(wq_buf.at[2 * g], rq_sems.at[2 * g])
            wait_sem(wq_buf.at[2 * g + 1], rq_sems.at[2 * g + 1])

        wait_sem(kv_buf.at[pl.ds(2 * g, 2)], ld_sems.at[L_KV + g])
        attn_group(g)
        return carry

    lax.fori_loop(0, 4, loop_body, 0)

    lo_u = lax.broadcasted_iota(jnp.int32, (ROWS // 2, 128), 1) < 64
    c6 = pltpu.bitcast(ctx_buf[6], jnp.uint32)
    c7 = pltpu.bitcast(ctx_buf[7], jnp.uint32)
    cl_buf[0] = pltpu.bitcast(jnp.where(lo_u, c6, c7), BF16)
    cl_buf[1] = pltpu.bitcast(jnp.where(lo_u, c7, c6), BF16)
    wait_sem(head_buf, send_sems.at[S_HEAD])
    wait_sem(wq_buf.at[pl.ds(0, 2), tail_rows], send_sems.at[S_WQ1])
    wait_sem(wq_buf.at[pl.ds(0, 4)], send_sems.at[S_WQ])
    wait_sem(wo_buf.at[4], ro_sems.at[2])
    wait_sem(wo_buf.at[5], ro_sems.at[3])
    out_ref[...] += _nn(ctx_buf[4], wo_buf[4]) + _nn(ctx_buf[5], wo_buf[5])
    for c in range(NO_CHUNK - 1):
        cols = pl.ds(c * CW, CW)
        wait_sem(wo_buf.at[6, :, cols], ro_sems.at[4 + 2 * c])
        wait_sem(wo_buf.at[7, :, cols], ro_sems.at[5 + 2 * c])
        for r in range(2):
            rows = pl.ds(r * 256, 256)
            out_ref[rows, cols] += (_nn(ctx_buf[6, rows, :], wo_buf[6, :, cols])
                                    + _nn(ctx_buf[7, rows, :], wo_buf[7, :, cols]))
    for j in range(2):
        for d in range(2):
            half = pl.ds(64 * ((d + j) % 2), 64)
            wait_sem(wl_buf.at[j, half], ro_sems.at[4 + 2 * (NO_CHUNK - 1 + j) + d])
        for r in range(4):
            rows = pl.ds(r * 128, 128)
            out_ref[rows, lcols] += _nn(cl_buf[j, rows, :], wl_buf[j])

    wait_sem(wo_buf.at[pl.ds(0, 6)], send_sems.at[S_WO])


def _compiler_params():
    kw = dict(collective_id=0, vmem_limit_bytes=48 * 1024 * 1024)
    for name in ("disable_semaphore_checks", "disable_bounds_checks"):
        if hasattr(pltpu.CompilerParams, name):
            kw[name] = True
    return pltpu.CompilerParams(**kw)


def pallas_dist_sparse_attn_blocksparse_qseq_b2_sq256_skv256_hq4_dh64_kernel(x, Wq, K_ext, V_ext, Wo):
    kt = jnp.transpose(K_ext, (0, 2, 3, 1)).reshape(B, 8, 128, 256)
    vt = jnp.transpose(V_ext, (0, 2, 3, 1)).reshape(B, 8, 128, 256)
    out = pl.pallas_call(
        _body,
        out_shape=jax.ShapeDtypeStruct((ROWS, DM), F32),
        in_specs=[pl.BlockSpec(memory_space=pl.ANY)] * 5,
        out_specs=pl.BlockSpec(memory_space=pltpu.VMEM),
        scratch_shapes=[
            pltpu.VMEM((ROWS, DM), F32),
            pltpu.VMEM((ROWS, DM), BF16),
            pltpu.VMEM((DM, 256), F32),
            pltpu.VMEM((256, DM), F32),
            pltpu.VMEM((8, DM, 128), BF16),
            pltpu.VMEM((8, 128, DM), BF16),
            pltpu.VMEM((8, 2, B, 128, 256), F32),
            pltpu.VMEM((8, ROWS, 128), BF16),
            pltpu.VMEM((4, 4, 128, 128), BF16),
            pltpu.VMEM((4, 4, 128, 128), BF16),
            pltpu.VMEM((2, HEAD, 128), F32),
            pltpu.VMEM((2, 128, 128), BF16),
            pltpu.VMEM((2, ROWS, 128), BF16),
            pltpu.SemaphoreType.DMA((L_KV + 4,)),
            pltpu.SemaphoreType.DMA((4,)),
            pltpu.SemaphoreType.DMA((8,)),
            pltpu.SemaphoreType.DMA((6 + 2 * NO_CHUNK,)),
            pltpu.SemaphoreType.REGULAR,
        ],
        compiler_params=_compiler_params(),
    )(x.reshape(ROWS, DM), Wq, kt, vt, Wo)
    return out.reshape(B, SQ, DM)
```
